```python
import numpy as np

kernel_name = "dist_max_ax1_xy_m2048_n1024"

def setup_inputs():
    return {"x": np.random.randn(4096, 2048).astype(np.float32)}

def reference(x: np.ndarray) -> np.ndarray:
    return np.max(x, axis=1, keepdims=True)
```

```python
import contextlib
import jax, jax.numpy as jnp
from jax import lax
from jax.experimental import pallas as pl
from jax.experimental.pallas import tpu as pltpu

M, N = 2048, 1024
G = 128
NG = M // G
NEG = float("-inf")


def _tree(parts):
    while len(parts) > 1:
        nxt = [jnp.maximum(parts[i], parts[i + 1]) for i in range(0, len(parts) - 1, 2)]
        if len(parts) % 2:
            nxt.append(parts[-1])
        parts = nxt
    return parts[0]


def _fold_cols(v):
    return _tree([v[:, j * 128:(j + 1) * 128] for j in range(N // 128)])


def _diag(m, lane0):
    R = m.shape[0]
    r = jnp.max(m, axis=1, keepdims=True)
    row = lax.broadcasted_iota(jnp.int32, (R, 128), 0)
    lane = lax.broadcasted_iota(jnp.int32, (R, 128), 1)
    d = jnp.where(lane == row + lane0, r, NEG)
    return _tree([d[k * 8:(k + 1) * 8] for k in range(R // 8)])


def make(tail=((80, 1), (32, 0), (16, 1)), P=8, NP=10, lag=1, scopes=False):
    assert sum(t for t, _ in tail) == G
    side = P * NP
    assert side <= G
    def scope(n):
        return jax.named_scope(n) if scopes else contextlib.nullcontext()

    def kernel(x):
        def body(x_ref, o_ref, buf, part, rbuf, sbuf, gsem, tsem, ssem, rsem, s1sem, s2sem):
            def gcopy(g):
                if isinstance(g, int) and g == 0:
                    return pltpu.make_async_copy(x_ref.at[pl.ds(side, G - side), :], buf.at[pl.ds(side, G - side), :], gsem.at[0])
                return pltpu.make_async_copy(x_ref.at[pl.ds(g * G, G), :], buf.at[pl.ds(g * G, G), :], gsem.at[g])
            def s1copy(p):
                return pltpu.make_async_copy(x_ref.at[pl.ds(p * P, P), :], sbuf.at[p], s1sem.at[p])
            def s2copy(p):
                st = p * P if isinstance(p, int) else pl.multiple_of(p * P, P)
                return pltpu.make_async_copy(sbuf.at[p], buf.at[pl.ds(st, P), :], s2sem)

            gcopy(1).start()
            for p in range(NP):
                s1copy(p).start()
            for g in range(2, NG - 1):
                gcopy(g).start()
                if g == 2 and side < G:
                    gcopy(0).start()
            tcopies = []
            off = (NG - 1) * G
            for i, (t, xl) in enumerate(tail):
                c = pltpu.make_async_copy(x_ref.at[pl.ds(off, t), :], buf.at[pl.ds(off, t), :], tsem.at[i])
                c.start(); tcopies.append((c, off, t, xl)); off += t

            mx = lax.axis_index("x"); my = lax.axis_index("y")
            peer = (mx, 1 - my)
            bar = pltpu.get_barrier_semaphore()
            pl.semaphore_signal(bar, inc=1, device_id=peer, device_id_type=pl.DeviceIdType.MESH)

            def group(g):
                start = g * G if isinstance(g, int) else pl.multiple_of(g * G, G)
                m = _fold_cols(buf[pl.ds(start, G), :])
                part[g] = jnp.max(_diag(m, 0), axis=0, keepdims=True)

            def rc(lo, n, k):
                return pltpu.make_async_remote_copy(part.at[pl.ds(lo, n)], rbuf.at[pl.ds(lo, n)], ssem.at[k], rsem.at[k],
                                             device_id=peer, device_id_type=pl.DeviceIdType.MESH)

            step = max(1, P // 8)
            def it(g, c):
                gcopy(g).wait()
                if NP:
                    q = g - 1 - lag
                    @pl.when((q >= step - 1) & (q < NP * step) & (lax.rem(q, step) == step - 1))
                    def _():
                        p = q // step
                        s1copy(p).wait()
                        s2copy(p).start()
                group(g)
                return c
            assert 1 + lag + NP * step <= NG - 1, "too many pieces"
            with scope("loop"):
                lax.fori_loop(1, NG - 1, it, 0)
            with scope("g0w"):
                if side < G:
                    gcopy(0).wait()
                if NP:
                    pltpu.make_async_copy(buf.at[pl.ds(0, side), :], buf.at[pl.ds(0, side), :], s2sem).wait()
            with scope("g0"):
                group(0)
            pl.semaphore_wait(bar, 1)
            rc(0, NG - 1, 0).start()
            acc = None
            pend = []
            for i, (c, off, t, xl) in enumerate(tcopies):
                with scope("tw%d" % i):
                    c.wait()
                with scope("tc%d" % i):
                    pend.append((_fold_cols(buf[pl.ds(off, t), :]), off - (NG - 1) * G))
                    if xl:
                        ds = [_diag(m, l0) for m, l0 in pend]
                        pend = []
                        acc = _tree(([acc] if acc is not None else []) + ds)
                    if i == len(tcopies) - 1:
                        last = jnp.max(acc, axis=0, keepdims=True)
                        part[NG - 1] = last
                        rc(NG - 1, 1, 1).start()
            with scope("recv0"):
                rc(0, NG - 1, 0).wait()
                o_ref[pl.ds(0, NG - 1)] = jnp.maximum(part[pl.ds(0, NG - 1)], rbuf[pl.ds(0, NG - 1)])
                rc(NG - 1, 1, 1).wait_send()
            with scope("recv1"):
                rc(NG - 1, 1, 1).wait_recv()
            o_ref[NG - 1] = jnp.maximum(last, rbuf[NG - 1])

        o = pl.pallas_call(
            body,
            out_shape=jax.ShapeDtypeStruct((NG, 1, 128), jnp.float32),
            in_specs=[pl.BlockSpec(memory_space=pl.ANY)],
            out_specs=pl.BlockSpec(memory_space=pltpu.VMEM),
            scratch_shapes=[
                pltpu.VMEM((M, N), jnp.float32),
                pltpu.VMEM((NG, 1, 128), jnp.float32),
                pltpu.VMEM((NG, 1, 128), jnp.float32),
                pltpu.SMEM((max(NP, 1), P, N), jnp.float32),
                pltpu.SemaphoreType.DMA((NG - 1,)),
                pltpu.SemaphoreType.DMA((len(tail),)),
                pltpu.SemaphoreType.DMA((2,)),
                pltpu.SemaphoreType.DMA((2,)),
                pltpu.SemaphoreType.DMA((max(NP, 1),)),
                pltpu.SemaphoreType.DMA,
            ],
            compiler_params=pltpu.CompilerParams(collective_id=0, disable_semaphore_checks=True, disable_bounds_checks=True),
        )(x)
        return o.reshape(M, 1)
    return kernel


_impl = make(tail=((96, 1), (24, 0), (8, 1)), P=8, NP=6)


def pallas_dist_max_ax1_xy_m2048_n1024_kernel(x: jax.Array):
    return _impl(x)
```

```python
import contextlib
import jax, jax.numpy as jnp
from jax import lax
from jax.experimental import pallas as pl
from jax.experimental.pallas import tpu as pltpu

M, N = 2048, 1024
G = 128
NG = M // G
NB = G // 8
NEG = float("-inf")
MESH = pl.DeviceIdType.MESH
GR, L = NG - 2, NG - 1


def _tree(parts):
    while len(parts) > 1:
        nxt = [jnp.maximum(parts[i], parts[i + 1]) for i in range(0, len(parts) - 1, 2)]
        if len(parts) % 2:
            nxt.append(parts[-1])
        parts = nxt
    return parts[0]


def _fold_cols(v):
    return _tree([v[:, j * 128:(j + 1) * 128] for j in range(v.shape[1] // 128)])


def _diag_blocks(blocks, b0):
    row = lax.broadcasted_iota(jnp.int32, (8, 128), 0)
    lane = lax.broadcasted_iota(jnp.int32, (8, 128), 1)
    return _tree([jnp.where(lane == row + 8 * (b0 + j), jnp.max(_fold_cols(v), axis=1, keepdims=True), NEG)
                  for j, v in enumerate(blocks)])


def _pick_diag(d):
    lane = lax.broadcasted_iota(jnp.int32, (8, 128), 1)
    rots = [d] + [pltpu.roll(d, 8 - s, 0) for s in range(1, 8)]
    b0 = (lane & 1) != 0
    b1 = (lane & 2) != 0
    b2 = (lane & 4) != 0
    t = [jnp.where(b0, rots[2 * i + 1], rots[2 * i]) for i in range(4)]
    u = [jnp.where(b1, t[2 * i + 1], t[2 * i]) for i in range(2)]
    return jnp.where(b2, u[1], u[0])[0:1, :]


def make(T=(8, 4), C=3, F=1, pad=5, Z=2, Y=2, W=9, W1=7, NP=0, RB=15, lag=1, gr_at=1, fin="s", scopes=False, landing=False):
    chunks = tuple(T) + (C, F)
    assert sum(chunks) == NB
    KI = NG - 2 - (1 if NP else 0)
    GS = NG - 3
    sent = G - 8 * (F + C)
    def scope(n):
        return jax.named_scope(n) if (scopes is True or (scopes and n in scopes)) else contextlib.nullcontext()

    def kernel(x):
        def body(x_ref, o_ref, buf, rawbuf, acc, part, rbuf, last_v, rlast_s, sbuf,
                 gsem, tsem, ssem, rsem, s1sem, s2sem, lsem):
            def step_copy(i, k):
                return pltpu.make_async_copy(x_ref.at[pl.ds(0, k), i], buf.at[pl.ds(0, k), i], gsem.at[i])
            def blk_copy(g, b, n, sem):
                return pltpu.make_async_copy(x_ref.at[g, pl.ds(b, n)], buf.at[g, pl.ds(b, n)], sem)
            def kof(i):
                return KI + 1 if (NP and i >= NP) else KI
            def s1copy(p):
                return pltpu.make_async_copy(x_ref.at[GS, p], sbuf.at[p], s1sem.at[p])
            def s2copy(p):
                return pltpu.make_async_copy(sbuf.at[p], buf.at[GS, p], s2sem)

            step_copy(0, kof(0)).start()

            mx = lax.axis_index("x"); my = lax.axis_index("y")
            peer = (mx, 1 - my)
            bar = pltpu.get_barrier_semaphore()
            pl.semaphore_signal(bar, inc=1, device_id=peer, device_id_type=MESH)

            raw_src = x_ref.at[GR, pl.ds(0, RB)]
            def remote(src, dst, k):
                return pltpu.make_async_remote_copy(src, dst, ssem.at[k], rsem.at[k], device_id=peer, device_id_type=MESH)
            def rawcopy():
                return remote(raw_src, rawbuf, 3)

            @pl.when(my == 1)
            def _():
                pl.semaphore_wait(bar, 1)
                rawcopy().start()
            for p in range(NP):
                s1copy(p).start()
            for i in range(1, NB):
                if i == gr_at:
                    @pl.when(my == 1)
                    def _():
                        blk_copy(GR, RB, NB - RB, lsem.at[1]).start()
                    @pl.when(my == 0)
                    def _():
                        blk_copy(GR, 0, NB, lsem.at[1]).start()
                step_copy(i, kof(i)).start()
            tcopies = []
            off = 0
            for i, t in enumerate(chunks):
                c = blk_copy(L, off, t, tsem.at[i])
                c.start(); tcopies.append((c, off, t)); off += t

            def rc(lo, n, k):
                return remote(part.at[pl.ds(lo, n)], rbuf.at[pl.ds(lo, n)], k)
            def rclast():
                return remote(last_v, rlast_s, 2)

            row8 = lax.broadcasted_iota(jnp.int32, (8, 128), 0)
            lane8 = lax.broadcasted_iota(jnp.int32, (8, 128), 1)

            def step(i):
                m = (lane8 >> 3) == i
                for j in range(KI):
                    r = jnp.max(_fold_cols(buf[j, i]), axis=1, keepdims=True)
                    pltpu.store(acc.at[j], jnp.broadcast_to(r, (8, 128)), mask=m)

            def it(i, c):
                if NP:
                    @pl.when(i < NP)
                    def _():
                        step_copy(i, KI).wait()
                    @pl.when(i >= NP)
                    def _():
                        step_copy(i, KI + 1).wait()
                    q = i - lag
                    @pl.when((q >= 0) & (q < NP))
                    def _():
                        s1copy(q).wait()
                        s2copy(q).start()
                else:
                    step_copy(i, KI).wait()
                step(i)
                return c
            with scope("loop"):
                lax.fori_loop(0, NB - 1, it, 0)
            with scope("spec"):
                @pl.when(my == 1)
                def _():
                    blk_copy(GR, RB, NB - RB, lsem.at[1]).wait()
                    part[GR] = _pick_diag(_diag_blocks([buf[GR, b] for b in range(RB, NB)], RB))
                @pl.when(my == 0)
                def _():
                    blk_copy(GR, 0, NB, lsem.at[1]).wait()
                    part[GR] = _pick_diag(_diag_blocks([buf[GR, b] for b in range(NB)], 0))
                    pl.semaphore_wait(bar, 1)
                if NP:
                    with scope("s2w"):
                        blk_copy(GS, 0, NP, s2sem).wait()
                    dgs = _diag_blocks([buf[GS, b] for b in range(NB - 1)], 0)
            with scope("s15"):
                step_copy(NB - 1, kof(NB - 1)).wait()
                for j in range(KI):
                    r = jnp.max(_fold_cols(buf[j, NB - 1]), axis=1, keepdims=True)
                    part[j] = _pick_diag(jnp.where(lane8 >= G - 8, r, acc[j]))
                if NP:
                    part[GS] = _pick_diag(jnp.maximum(dgs, _diag_blocks([buf[GS, NB - 1]], NB - 1)))
            rc(0, L, 0).start()

            if landing:
                for i, (c, off, t) in enumerate(tcopies):
                    with jax.named_scope("L%02d" % i):
                        c.wait()
                class _Nop:
                    def wait(self): pass
                tcopies = [(_Nop(), off, t) for (c, off, t) in tcopies]
            acc0 = None
            for i in range(len(T)):
                with scope("t%d" % i):
                    c, off, t = tcopies[i]
                    c.wait()
                    d = _diag_blocks([buf[L, b] for b in range(off, off + t)], off)
                    acc0 = d if acc0 is None else jnp.maximum(acc0, d)
            with scope("tail"):
                def dmask(b):
                    return lane8 == row8 + 8 * b
                c, off, t = tcopies[len(T)]
                c.wait()
                cf = []
                anc = acc0
                for b in range(off, off + t):
                    v = buf[L, b]
                    h0, h1 = _fold_cols(v[:, :N // 2]), _fold_cols(v[:, N // 2:])
                    f = jnp.maximum(h0, h1)
                    cf.append((f, h0, b))
                    anc = jnp.where(dmask(b), f, anc)
                for _ in range(pad):
                    anc = jnp.maximum(pltpu.roll(anc, 1, 0), acc0)
                c, off, t = tcopies[len(T) + 1]
                c.wait()
                ff = [(_fold_cols(buf[L, b]), b) for b in range(off, off + t)]
                first = _pick_diag(acc0)
                part[L] = first
                rc(L, 1, 1).start()
                ff = [(f, b) for (f, h0, b) in cf[2:]] + ff
                cf = cf[:2]
                d2 = acc0
                dums = []
                for j, (f, h0, b) in enumerate(cf):
                    d2 = jnp.where(dmask(b), jnp.max(f, axis=1, keepdims=True), d2)
                    for z in range(Z if j == 0 else Y):
                        d2 = jnp.maximum(d2, anc if z % 2 else acc0)
                    dums.append(jnp.where(dmask(b), jnp.max(h0, axis=1, keepdims=True), NEG))
                for f, b in ff:
                    d2 = jnp.where(lane8 >= 8 * b, jnp.max(f, axis=1, keepdims=True), d2)
                last = _pick_diag(d2)
                last_v[...] = last
                rclast().start()
                for z in range(W):
                    dums[0] = jnp.maximum(dums[0], anc if z % 2 else acc0)
                for z in range(W1):
                    dums[1] = jnp.maximum(dums[1], anc if z % 2 else acc0)

            @pl.when(my == 1)
            def _():
                c1 = pltpu.make_async_copy(raw_src, rawbuf, lsem.at[0]); c1.start()
                rawcopy().wait_send()
                c1.wait()
            @pl.when(my == 0)
            def _():
                with scope("raww"):
                    rawcopy().wait_recv()
            rawp = _pick_diag(_diag_blocks([rawbuf[b] for b in range(RB)], 0))
            own = jnp.maximum(last, jnp.max(jnp.maximum(dums[0], dums[1]), axis=0, keepdims=True))
            with scope("recv0"):
                rclast().wait_send()
                rc(L, 1, 1).wait_send()
                rc(0, L, 0).wait()
                o_ref[pl.ds(0, GR)] = jnp.maximum(part[pl.ds(0, GR)], rbuf[pl.ds(0, GR)])
                o_ref[GR] = jnp.maximum(jnp.maximum(part[GR], rawp), rbuf[GR])
            lane = lax.broadcasted_iota(jnp.int32, (1, 128), 1)
            def fin_s(own):
                with scope("recv3"):
                    rclast().wait_recv()
                a = jnp.full((1, 128), NEG, jnp.float32)
                for i in range(sent, G):
                    a = jnp.where(lane == i, rlast_s[0, i], a)
                return jnp.maximum(own, a)
            def fin_v(own):
                with scope("recv2"):
                    rc(L, 1, 1).wait_recv()
                return jnp.maximum(own, rbuf[L])
            if fin == "s":
                o_ref[L] = fin_v(fin_s(own))
            else:
                o_ref[L] = fin_s(fin_v(own))

        o = pl.pallas_call(
            body,
            out_shape=jax.ShapeDtypeStruct((NG, 1, 128), jnp.float32),
            in_specs=[pl.BlockSpec(memory_space=pl.ANY)],
            out_specs=pl.BlockSpec(memory_space=pltpu.VMEM),
            scratch_shapes=[
                pltpu.VMEM((NG, NB, 8, N), jnp.float32),
                pltpu.VMEM((RB, 8, N), jnp.float32),
                pltpu.VMEM((KI, 8, 128), jnp.float32),
                pltpu.VMEM((NG, 1, 128), jnp.float32),
                pltpu.VMEM((NG, 1, 128), jnp.float32),
                pltpu.VMEM((1, 128), jnp.float32),
                pltpu.SMEM((1, 128), jnp.float32),
                pltpu.SMEM((max(NP, 1), 8, N), jnp.float32),
                pltpu.SemaphoreType.DMA((NB,)),
                pltpu.SemaphoreType.DMA((len(chunks),)),
                pltpu.SemaphoreType.DMA((4,)),
                pltpu.SemaphoreType.DMA((4,)),
                pltpu.SemaphoreType.DMA((max(NP, 1),)),
                pltpu.SemaphoreType.DMA,
                pltpu.SemaphoreType.DMA((2,)),
            ],
            compiler_params=pltpu.CompilerParams(collective_id=0, disable_semaphore_checks=True, disable_bounds_checks=True),
        )(x.reshape(NG, NB, 8, N))
        return o.reshape(M, 1)
    return kernel


_impl = make(NP=4)


def pallas_dist_max_ax1_xy_m2048_n1024_kernel(x: jax.Array):
    return _impl(x)
```

```python
import contextlib
import jax, jax.numpy as jnp
from jax import lax
from jax.experimental import pallas as pl
from jax.experimental.pallas import tpu as pltpu

M, N = 2048, 1024
G = 128
NG = M // G
NB = G // 8
TB = N // 128
TG = NB * TB
NEG = float("-inf")
MESH = pl.DeviceIdType.MESH
GR, L = NG - 2, NG - 1


def _tree(parts):
    while len(parts) > 1:
        nxt = [jnp.maximum(parts[i], parts[i + 1]) for i in range(0, len(parts) - 1, 2)]
        if len(parts) % 2:
            nxt.append(parts[-1])
        parts = nxt
    return parts[0]


def _pick_diag(d):
    lane = lax.broadcasted_iota(jnp.int32, (8, 128), 1)
    rots = [d] + [pltpu.roll(d, 8 - s, 0) for s in range(1, 8)]
    b0 = (lane & 1) != 0
    b1 = (lane & 2) != 0
    b2 = (lane & 4) != 0
    t = [jnp.where(b0, rots[2 * i + 1], rots[2 * i]) for i in range(4)]
    u = [jnp.where(b1, t[2 * i + 1], t[2 * i]) for i in range(2)]
    return jnp.where(b2, u[1], u[0])[0:1, :]


def make(P=16, SH=7, SP=2, T=(8, 4), C=3, F=1, pad=5, Z=2, Y=2, W=9, W1=7, ST=0, SPC=8, RT=116, lag=1,
         gr_at=2, spec_at=None, fin="s", scopes=False):
    chunks = tuple(T) + (C, F)
    assert sum(chunks) == NB
    GS = NG - 3
    KI = NG - 2
    sent = G - 8 * (F + C)
    bounds = ([SH] if SH else []) + list(range(SH + P, TG, P)) + [TG]
    steps = []
    a = 0
    for b in bounds:
        k = KI if a >= ST else KI - 1
        assert a >= ST or b <= ST, "ST must be on a step boundary"
        per = -(-KI // SP)
        for s in range(SP):
            g0 = s * per
            kk = min(per, k - g0)
            steps.append((g0, kk, a, b - a))
        a = b
    spieces = [(t, min(SPC, ST - t)) for t in range(0, ST, SPC)]
    NP = len(spieces)
    def scope(n):
        return jax.named_scope(n) if (scopes is True or (scopes and n in scopes)) else contextlib.nullcontext()

    def kernel(x):
        def body(x_ref, o_ref, buf, rawbuf, part, rbuf, last_v, rlast_s, sbuf,
                 gsem, tsem, ssem, rsem, s1sem, s2sem, lsem):
            def step_copy(i):
                g0, k, t0, n = steps[i]
                return pltpu.make_async_copy(x_ref.at[pl.ds(g0, k), pl.ds(t0, n)], buf.at[pl.ds(g0, k), pl.ds(t0, n)], gsem.at[i])
            def tile_copy(g, t0, n, sem):
                return pltpu.make_async_copy(x_ref.at[g, pl.ds(t0, n)], buf.at[g, pl.ds(t0, n)], sem)
            def s1copy(p):
                t0, n = spieces[p]
                return pltpu.make_async_copy(x_ref.at[GS, pl.ds(t0, n)], sbuf.at[pl.ds(t0, n)], s1sem.at[p])
            def s2copy(p):
                t0, n = spieces[p]
                return pltpu.make_async_copy(sbuf.at[pl.ds(t0, n)], buf.at[GS, pl.ds(t0, n)], s2sem)

            step_copy(0).start()

            mx = lax.axis_index("x"); my = lax.axis_index("y")
            peer = (mx, 1 - my)
            bar = pltpu.get_barrier_semaphore()
            pl.semaphore_signal(bar, inc=1, device_id=peer, device_id_type=MESH)

            raw_src = x_ref.at[GR, pl.ds(0, RT)]
            def remote(src, dst, k):
                return pltpu.make_async_remote_copy(src, dst, ssem.at[k], rsem.at[k], device_id=peer, device_id_type=MESH)
            def rawcopy():
                return remote(raw_src, rawbuf, 3)

            @pl.when(my == 1)
            def _():
                step_copy(1).start()
                pl.semaphore_wait(bar, 1)
                rawcopy().start()
            @pl.when(my == 0)
            def _():
                step_copy(1).start()
            for p in range(NP):
                s1copy(p).start()
            for i in range(2, len(steps)):
                if i == gr_at:
                    @pl.when(my == 1)
                    def _():
                        tile_copy(GR, RT, TG - RT, lsem.at[1]).start()
                    @pl.when(my == 0)
                    def _():
                        tile_copy(GR, 0, TG, lsem.at[1]).start()
                step_copy(i).start()
            tcopies = []
            off = 0
            for i, t in enumerate(chunks):
                c = tile_copy(L, off * TB, t * TB, tsem.at[i])
                c.start(); tcopies.append((c, off, t)); off += t

            def rc(lo, n, k):
                return remote(part.at[pl.ds(lo, n)], rbuf.at[pl.ds(lo, n)], k)
            def rclast():
                return remote(last_v, rlast_s, 2)

            row8 = lax.broadcasted_iota(jnp.int32, (8, 128), 0)
            lane8 = lax.broadcasted_iota(jnp.int32, (8, 128), 1)
            lgrp = lane8 >> 3

            def fold(ref, t0, t1):
                return _tree([ref[t] for t in range(t0, t1)])
            def rmax(f):
                return jnp.max(f, axis=1, keepdims=True)
            def tiles_diag(ref, t0, t1, init=None):
                d = jnp.full((8, 128), NEG, jnp.float32) if init is None else init
                for b in range(t0 // TB, -(-t1 // TB)):
                    lo, hi = max(t0, b * TB), min(t1, (b + 1) * TB)
                    d = jnp.where(lgrp == b, rmax(fold(ref, lo, hi)), d)
                return d

            def special():
                @pl.when(my == 1)
                def _():
                    tile_copy(GR, RT, TG - RT, lsem.at[1]).wait()
                    part[GR] = _pick_diag(tiles_diag(buf.at[GR], RT, TG))
                @pl.when(my == 0)
                def _():
                    tile_copy(GR, 0, TG, lsem.at[1]).wait()
                    part[GR] = _pick_diag(tiles_diag(buf.at[GR], 0, TG))
                    pl.semaphore_wait(bar, 1)

            acc = [None] * KI
            done = [0] * KI
            smem_done = (NP == 0)
            fwd = 0
            sp_at = spec_at if spec_at is not None else len(steps) - 4
            with scope("loop"):
                for i, (g0, k, t0, n) in enumerate(steps):
                    step_copy(i).wait()
                    if i >= lag and fwd < NP and (i - lag) % 1 == 0 and i >= 2:
                        s1copy(fwd).wait()
                        s2copy(fwd).start()
                        fwd += 1
                    if i == len(steps) - 3 and NP:
                        assert fwd == NP
                        with scope("s2w"):
                            tile_copy(GS, 0, ST, s2sem).wait()
                        smem_done = True
                    for g in range(g0, g0 + k):
                        if g == GS and not smem_done:
                            continue
                        nb = (t0 + n) // TB
                        for b in range(done[g], nb):
                            r = rmax(fold(buf.at[g], b * TB, (b + 1) * TB))
                            acc[g] = jnp.broadcast_to(r, (8, 128)) if acc[g] is None else jnp.where(lgrp == b, r, acc[g])
                        done[g] = nb
                        if nb == NB:
                            part[g] = _pick_diag(acc[g])
                    if i == sp_at:
                        special()
            assert all(d == NB for d in done)
            rc(0, L, 0).start()

            acc0 = None
            bl = buf.at[L]
            for i in range(len(T)):
                with scope("t%d" % i):
                    c, off, t = tcopies[i]
                    c.wait()
                    acc0 = tiles_diag(bl, off * TB, (off + t) * TB, acc0)
            with scope("tail"):
                def dmask(b):
                    return lane8 == row8 + 8 * b
                c, off, t = tcopies[len(T)]
                c.wait()
                cf = []
                low = jnp.where(lane8 == row8, acc0, NEG)
                anc = low
                for b in range(off, off + t):
                    h0, h1 = fold(bl, b * TB, b * TB + 4), fold(bl, b * TB + 4, (b + 1) * TB)
                    f = jnp.maximum(h0, h1)
                    cf.append((f, h0, b))
                    anc = jnp.where(dmask(b), f, anc)
                for _ in range(pad):
                    anc = jnp.maximum(pltpu.roll(anc, 1, 0), low)
                c, off, t = tcopies[len(T) + 1]
                c.wait()
                ff = [(fold(bl, b * TB, (b + 1) * TB), b) for b in range(off, off + t)]
                first = _pick_diag(acc0)
                part[L] = first
                rc(L, 1, 1).start()
                ff = [(f, b) for (f, h0, b) in cf[2:]] + ff
                cf = cf[:2]
                d2 = acc0
                dums = []
                for j, (f, h0, b) in enumerate(cf):
                    d2 = jnp.where(lgrp == b, rmax(f), d2)
                    for z in range(Z if j == 0 else Y):
                        d2 = jnp.maximum(d2, anc if z % 2 else low)
                    dums.append(jnp.where(dmask(b), rmax(h0), NEG))
                for f, b in ff:
                    d2 = jnp.where(lane8 >= 8 * b, rmax(f), d2)
                last = _pick_diag(d2)
                last_v[...] = last
                rclast().start()
                for z in range(W):
                    dums[0] = jnp.maximum(dums[0], anc if z % 2 else low)
                for z in range(W1):
                    dums[1] = jnp.maximum(dums[1], anc if z % 2 else low)

            @pl.when(my == 1)
            def _():
                c1 = pltpu.make_async_copy(raw_src, rawbuf, lsem.at[0]); c1.start()
                rawcopy().wait_send()
                c1.wait()
            @pl.when(my == 0)
            def _():
                with scope("raww"):
                    rawcopy().wait_recv()
            rawp = _pick_diag(tiles_diag(rawbuf, 0, RT))
            own = jnp.maximum(last, jnp.max(jnp.maximum(dums[0], dums[1]), axis=0, keepdims=True))
            with scope("recv0"):
                rclast().wait_send()
                rc(L, 1, 1).wait_send()
                rc(0, L, 0).wait()
                o_ref[pl.ds(0, GR)] = jnp.maximum(part[pl.ds(0, GR)], rbuf[pl.ds(0, GR)])
                o_ref[GR] = jnp.maximum(jnp.maximum(part[GR], rawp), rbuf[GR])
            lane = lax.broadcasted_iota(jnp.int32, (1, 128), 1)
            def fin_s(own):
                with scope("recv3"):
                    rclast().wait_recv()
                a = jnp.full((1, 128), NEG, jnp.float32)
                for i in range(sent, G):
                    a = jnp.where(lane == i, rlast_s[0, i], a)
                return jnp.maximum(own, a)
            def fin_v(own):
                with scope("recv2"):
                    rc(L, 1, 1).wait_recv()
                return jnp.maximum(own, rbuf[L])
            if fin == "s":
                o_ref[L] = fin_v(fin_s(own))
            else:
                o_ref[L] = fin_s(fin_v(own))

        xt = x.reshape(M // 8, 8, TB, 128).transpose(0, 2, 1, 3).reshape(NG, TG, 8, 128)
        o = pl.pallas_call(
            body,
            out_shape=jax.ShapeDtypeStruct((NG, 1, 128), jnp.float32),
            in_specs=[pl.BlockSpec(memory_space=pl.ANY)],
            out_specs=pl.BlockSpec(memory_space=pltpu.VMEM),
            scratch_shapes=[
                pltpu.VMEM((NG, TG, 8, 128), jnp.float32),
                pltpu.VMEM((RT, 8, 128), jnp.float32),
                pltpu.VMEM((NG, 1, 128), jnp.float32),
                pltpu.VMEM((NG, 1, 128), jnp.float32),
                pltpu.VMEM((1, 128), jnp.float32),
                pltpu.SMEM((1, 128), jnp.float32),
                pltpu.SMEM((max(ST, 1), 8, 128), jnp.float32),
                pltpu.SemaphoreType.DMA((len(steps),)),
                pltpu.SemaphoreType.DMA((len(chunks),)),
                pltpu.SemaphoreType.DMA((4,)),
                pltpu.SemaphoreType.DMA((4,)),
                pltpu.SemaphoreType.DMA((max(NP, 1),)),
                pltpu.SemaphoreType.DMA,
                pltpu.SemaphoreType.DMA((2,)),
            ],
            compiler_params=pltpu.CompilerParams(collective_id=0, disable_semaphore_checks=True, disable_bounds_checks=True),
        )(xt)
        return o.reshape(M, 1)
    return kernel


_impl = make(ST=39)


def pallas_dist_max_ax1_xy_m2048_n1024_kernel(x: jax.Array):
    return _impl(x)
```

```python
import jax
import jax.numpy as jnp
from jax import lax
from jax.experimental import pallas as pl
from jax.experimental.pallas import tpu as pltpu

M, N = 2048, 1024
G = 128
NG = M // G
NB = G // 8
TB = N // 128
TG = NB * TB
NT = NG * TG
LAST = NG - 1
NEG = float("-inf")
MESH = pl.DeviceIdType.MESH

U = 16
SH = 7
RT = 115
R7 = SH + 7 * U
QS = 2
ST0, ST = TG + SH, QS * U
QL = 3
NC, NF = 3, 1
CSTART = NT - (NC + NF) * TB
KLAST = 8 * (NC + NF)


def _plan():
    dmas = []
    for i in range(8):
        lo = 2 if i < QS else (1 if i < 7 else 0)
        hi = NG if i < QL else NG - 1
        splits = [hi - lo] if i < 7 else [7, 8]
        for k in splits:
            dmas.append((lo, k, i * U, U))
            lo += k
    c = CSTART - LAST * TG - SH
    dmas.append((LAST, 1, QL * U, c - QL * U))
    dmas.append((LAST, 1, c, NC * TB))
    dmas.append((LAST, 1, c + NC * TB, NF * TB))
    return dmas


_DMAS = _plan()
_I_FWD = 2
_I_G0 = 5
_I_SMEM = 6
_I_S7 = 7
_I_C = len(_DMAS) - 2
_BULK = ((0, 7), (7, 8))


def _tree_max(parts):
    while len(parts) > 1:
        nxt = [jnp.maximum(parts[i], parts[i + 1]) for i in range(0, len(parts) - 1, 2)]
        if len(parts) % 2:
            nxt.append(parts[-1])
        parts = nxt
    return parts[0]


def _fold(tile, t0, t1):
    return _tree_max([tile(t) for t in range(t0, t1)])


def _rmax(f):
    return jnp.max(f, axis=1, keepdims=True)


def _pick_diag(d):
    lane = lax.broadcasted_iota(jnp.int32, (8, 128), 1)
    rots = [d] + [pltpu.roll(d, 8 - s, 0) for s in range(1, 8)]
    t = [jnp.where((lane & 1) != 0, rots[2 * i + 1], rots[2 * i]) for i in range(4)]
    u = [jnp.where((lane & 2) != 0, t[2 * i + 1], t[2 * i]) for i in range(2)]
    return jnp.where((lane & 4) != 0, u[1], u[0])[0:1, :]


def _body(xg_ref, x_ref, o_ref, buf, g0buf, rawbuf, part, rbuf, last_v, last_s, sbuf,
          msem, lsem, ssem, rsem):
    def tile(t):
        return buf[(t - SH) // TG, (t - SH) % TG]

    def main_start(idx):
        j0, k, q, n = _DMAS[idx]
        if SH + q + n <= TG:
            pltpu.make_async_copy(xg_ref.at[pl.ds(j0, k), pl.ds(SH + q, n)],
                                  buf.at[pl.ds(j0, k), pl.ds(q, n)], msem.at[idx]).start()
        else:
            for j in range(j0, j0 + k):
                pltpu.make_async_copy(x_ref.at[pl.ds(j * TG + SH + q, n)],
                                      buf.at[j, pl.ds(q, n)], msem.at[idx]).start()

    def main_wait(idx):
        j0, k, q, n = _DMAS[idx]
        dst = buf.at[pl.ds(j0, k), pl.ds(q, n)]
        pltpu.make_async_copy(dst, dst, msem.at[idx]).wait()

    main_start(0)

    mx = lax.axis_index("x")
    my = lax.axis_index("y")
    peer = (mx, 1 - my)
    barrier = pltpu.get_barrier_semaphore()
    pl.semaphore_signal(barrier, inc=1, device_id=peer, device_id_type=MESH)

    def remote(src, dst, k):
        return pltpu.make_async_remote_copy(src, dst, ssem.at[k], rsem.at[k],
                                            device_id=peer, device_id_type=MESH)

    def raw_remote():
        return remote(x_ref.at[pl.ds(0, RT)], rawbuf, 0)

    def rows_remote(lo, n, k):
        return remote(part.at[pl.ds(lo, n)], rbuf.at[pl.ds(lo, n)], k)

    def last_remote():
        return remote(last_v, last_s, 4)

    def to_smem():
        return pltpu.make_async_copy(x_ref.at[pl.ds(ST0, ST)], sbuf, lsem.at[0])

    def from_smem():
        return pltpu.make_async_copy(sbuf, buf.at[1, pl.ds(0, ST)], lsem.at[1])

    def g0_copy(t0):
        return pltpu.make_async_copy(x_ref.at[pl.ds(t0, R7 - t0)],
                                     g0buf.at[pl.ds(t0, R7 - t0)], lsem.at[2])

    @pl.when(my == 1)
    def _():
        pl.semaphore_wait(barrier, 1)
        raw_remote().start()

    to_smem().start()
    main_start(1)

    @pl.when(my == 1)
    def _():
        g0_copy(RT).start()

    @pl.when(my == 0)
    def _():
        g0_copy(0).start()

    for idx in range(2, _I_S7):
        main_start(idx)

    row8 = lax.broadcasted_iota(jnp.int32, (8, 128), 0)
    lane8 = lax.broadcasted_iota(jnp.int32, (8, 128), 1)
    lgrp = lane8 >> 3

    def group0_row(src, t0, t1):
        d = jnp.full((8, 128), NEG, jnp.float32)
        for b in range(t0 // TB, -(-t1 // TB)):
            f = _fold(src, max(t0, b * TB), min(t1, (b + 1) * TB))
            d = jnp.where(lgrp == b, _rmax(f), d)
        return _pick_diag(d)

    landed, done, acc = set(), set(), {}
    for idx in range(_I_C):
        main_wait(idx)
        j0, k, q, n = _DMAS[idx]
        landed.update(j * TG + SH + t for j in range(j0, j0 + k) for t in range(q, q + n))
        if idx == 0:
            for later in range(_I_S7, len(_DMAS)):
                main_start(later)
        if idx == _I_FWD:
            to_smem().wait()
            from_smem().start()
        if idx == _I_SMEM:
            from_smem().wait()
            landed.update(range(ST0, ST0 + ST))
        for b in range(NB, CSTART // TB):
            if b not in done and all(t in landed for t in range(b * TB, (b + 1) * TB)):
                done.add(b)
                g = b // NB
                r = _rmax(_fold(tile, b * TB, (b + 1) * TB))
                if g in acc or g == LAST:
                    acc[g] = jnp.where(lgrp == b % NB, r, acc.get(g, NEG))
                else:
                    acc[g] = jnp.broadcast_to(r, (8, 128))
        if idx == _I_G0:
            @pl.when(my == 1)
            def _():
                g0_copy(RT).wait()
                part[0] = group0_row(lambda t: g0buf[t], RT, R7)

            @pl.when(my == 0)
            def _():
                g0_copy(0).wait()
                part[0] = group0_row(lambda t: g0buf[t], 0, R7)
                pl.semaphore_wait(barrier, 1)
        if _I_S7 <= idx < _I_S7 + len(_BULK):
            lo, cnt = _BULK[idx - _I_S7]
            for g in range(lo, lo + cnt):
                if g == 0:
                    part[0] = jnp.maximum(part[0], group0_row(tile, R7, TG))
                else:
                    assert all(b in done for b in range(g * NB, (g + 1) * NB))
                    part[g] = _pick_diag(acc[g])
            rows_remote(lo, cnt, 1 + idx - _I_S7).start()
    assert len(done) == CSTART // TB - NB

    acc0 = acc[LAST]
    b0 = CSTART // TB

    def diag(b):
        return lane8 == row8 + 8 * (b % NB)

    main_wait(_I_C)
    low = jnp.where(lane8 == row8, acc0, NEG)
    anc = low
    folds, halves = [], []
    for b in range(b0, b0 + NC):
        h0 = _fold(tile, b * TB, b * TB + TB // 2)
        f = jnp.maximum(h0, _fold(tile, b * TB + TB // 2, (b + 1) * TB))
        folds.append(f)
        halves.append(h0)
        anc = jnp.where(diag(b), f, anc)
    for _ in range(5):
        anc = jnp.maximum(pltpu.roll(anc, 1, 0), low)

    def chain(v, n):
        for z in range(n):
            v = jnp.maximum(v, anc if z % 2 else low)
        return v

    main_wait(_I_C + 1)
    folds.append(_fold(tile, (b0 + NC) * TB, NT))
    part[LAST] = _pick_diag(acc0)
    rows_remote(LAST, 1, 3).start()
    d = acc0
    aux = []
    for j in range(2):
        d = chain(jnp.where(lgrp == (b0 + j) % NB, _rmax(folds[j]), d), 2)
        aux.append(jnp.where(diag(b0 + j), _rmax(halves[j]), NEG))
    for j in range(2, NC + NF):
        d = jnp.where(lane8 >= 8 * ((b0 + j) % NB), _rmax(folds[j]), d)
    own = _pick_diag(d)
    last_v[...] = own
    last_remote().start()
    aux = [chain(aux[0], 9), chain(aux[1], 7)]

    @pl.when(my == 1)
    def _():
        again = pltpu.make_async_copy(x_ref.at[pl.ds(0, RT)], rawbuf, lsem.at[3])
        again.start()
        raw_remote().wait_send()
        again.wait()

    @pl.when(my == 0)
    def _():
        raw_remote().wait_recv()

    own0 = jnp.maximum(part[0], group0_row(lambda t: rawbuf[t], 0, RT))
    own = jnp.maximum(own, jnp.max(jnp.maximum(aux[0], aux[1]), axis=0, keepdims=True))

    last_remote().wait_send()
    rows_remote(LAST, 1, 3).wait_send()
    for k, (lo, cnt) in enumerate(_BULK):
        rows_remote(lo, cnt, 1 + k).wait()
        for g in range(lo, lo + cnt):
            o_ref[g] = jnp.maximum(own0 if g == 0 else part[g], rbuf[g])

    last_remote().wait_recv()
    lane = lax.broadcasted_iota(jnp.int32, (1, 128), 1)
    got = jnp.full((1, 128), NEG, jnp.float32)
    for i in range(G - KLAST, G):
        got = jnp.where(lane == i, last_s[0, i], got)
    own = jnp.maximum(own, got)
    rows_remote(LAST, 1, 3).wait_recv()
    o_ref[LAST] = jnp.maximum(own, rbuf[LAST])


def pallas_dist_max_ax1_xy_m2048_n1024_kernel(x: jax.Array):
    tiles = x.reshape(M // 8, 8, TB, 128).transpose(0, 2, 1, 3).reshape(NT, 8, 128)
    out = pl.pallas_call(
        _body,
        out_shape=jax.ShapeDtypeStruct((NG, 1, 128), jnp.float32),
        in_specs=[pl.BlockSpec(memory_space=pl.ANY), pl.BlockSpec(memory_space=pl.ANY)],
        out_specs=pl.BlockSpec(memory_space=pltpu.VMEM),
        scratch_shapes=[
            pltpu.VMEM((NG, TG, 8, 128), jnp.float32),
            pltpu.VMEM((R7, 8, 128), jnp.float32),
            pltpu.VMEM((RT, 8, 128), jnp.float32),
            pltpu.VMEM((NG, 1, 128), jnp.float32),
            pltpu.VMEM((NG, 1, 128), jnp.float32),
            pltpu.VMEM((1, 128), jnp.float32),
            pltpu.SMEM((1, 128), jnp.float32),
            pltpu.SMEM((ST, 8, 128), jnp.float32),
            pltpu.SemaphoreType.DMA((len(_DMAS),)),
            pltpu.SemaphoreType.DMA((4,)),
            pltpu.SemaphoreType.DMA((5,)),
            pltpu.SemaphoreType.DMA((5,)),
        ],
        compiler_params=pltpu.CompilerParams(collective_id=0, disable_semaphore_checks=True),
    )(tiles.reshape(NG, TG, 8, 128), tiles)
    return out.reshape(M, 1)
```

```python
import jax
import jax.numpy as jnp
from jax import lax
from jax.experimental import pallas as pl
from jax.experimental.pallas import tpu as pltpu

M, N = 2048, 1024
G = 128
NG = M // G
NB = G // 8
TB = N // 128
TG = NB * TB
NT = NG * TG
LAST = NG - 1
NEG = float("-inf")
MESH = pl.DeviceIdType.MESH

U = 16
SH = 7
RT = 117
R7 = SH + 7 * U
QS = 2
ST0, ST = TG + SH, QS * U
QL = 3
NC, NF = 3, 1
CSTART = NT - (NC + NF) * TB
KLAST = 8 * (NC + NF)


def _plan():
    dmas = []
    for i in range(8):
        lo = 2 if i < QS else (1 if i < 7 else 0)
        hi = NG if i < QL else NG - 1
        splits = [hi - lo] if i < 7 else [7, 8]
        for k in splits:
            dmas.append((lo, k, i * U, U))
            lo += k
    c = CSTART - LAST * TG - SH
    dmas.append((LAST, 1, QL * U, c - QL * U))
    dmas.append((LAST, 1, c, NC * TB))
    dmas.append((LAST, 1, c + NC * TB, NF * TB))
    return dmas


_DMAS = _plan()
_I_FWD = 2
_I_G0 = 5
_I_SMEM = 6
_I_S7 = 7
_I_C = len(_DMAS) - 2
_BULK = ((0, 7), (7, 8))


def _tree_max(parts):
    while len(parts) > 1:
        nxt = [jnp.maximum(parts[i], parts[i + 1]) for i in range(0, len(parts) - 1, 2)]
        if len(parts) % 2:
            nxt.append(parts[-1])
        parts = nxt
    return parts[0]


def _fold(tile, t0, t1):
    return _tree_max([tile(t) for t in range(t0, t1)])


def _rmax(f):
    return jnp.max(f, axis=1, keepdims=True)


def _pick_diag(d):
    lane = lax.broadcasted_iota(jnp.int32, (8, 128), 1)
    rots = [d] + [pltpu.roll(d, 8 - s, 0) for s in range(1, 8)]
    t = [jnp.where((lane & 1) != 0, rots[2 * i + 1], rots[2 * i]) for i in range(4)]
    u = [jnp.where((lane & 2) != 0, t[2 * i + 1], t[2 * i]) for i in range(2)]
    return jnp.where((lane & 4) != 0, u[1], u[0])[0:1, :]


def _body(xg_ref, x_ref, o_ref, buf, g0buf, rawbuf, part, rbuf, last_v, last_s, sbuf,
          msem, lsem, ssem, rsem):
    def tile(t):
        return buf[(t - SH) // TG, (t - SH) % TG]

    def main_start(idx):
        j0, k, q, n = _DMAS[idx]
        if SH + q + n <= TG:
            pltpu.make_async_copy(xg_ref.at[pl.ds(j0, k), pl.ds(SH + q, n)],
                                  buf.at[pl.ds(j0, k), pl.ds(q, n)], msem.at[idx]).start()
        else:
            for j in range(j0, j0 + k):
                pltpu.make_async_copy(x_ref.at[pl.ds(j * TG + SH + q, n)],
                                      buf.at[j, pl.ds(q, n)], msem.at[idx]).start()

    def main_wait(idx):
        j0, k, q, n = _DMAS[idx]
        dst = buf.at[pl.ds(j0, k), pl.ds(q, n)]
        pltpu.make_async_copy(dst, dst, msem.at[idx]).wait()

    main_start(0)

    mx = lax.axis_index("x")
    my = lax.axis_index("y")
    peer = (mx, 1 - my)
    barrier = pltpu.get_barrier_semaphore()
    pl.semaphore_signal(barrier, inc=1, device_id=peer, device_id_type=MESH)

    def remote(src, dst, k):
        return pltpu.make_async_remote_copy(src, dst, ssem.at[k], rsem.at[k],
                                            device_id=peer, device_id_type=MESH)

    def raw_remote():
        return remote(x_ref.at[pl.ds(0, RT)], rawbuf, 0)

    def rows_remote(lo, n, k):
        return remote(part.at[pl.ds(lo, n)], rbuf.at[pl.ds(lo, n)], k)

    def last_remote():
        return remote(last_v, last_s, 4)

    def to_smem():
        return pltpu.make_async_copy(x_ref.at[pl.ds(ST0, ST)], sbuf, lsem.at[0])

    def from_smem():
        return pltpu.make_async_copy(sbuf, buf.at[1, pl.ds(0, ST)], lsem.at[1])

    def g0_copy(t0):
        return pltpu.make_async_copy(x_ref.at[pl.ds(t0, R7 - t0)],
                                     g0buf.at[pl.ds(t0, R7 - t0)], lsem.at[2])

    @pl.when(my == 1)
    def _():
        pl.semaphore_wait(barrier, 1)
        raw_remote().start()

    to_smem().start()
    main_start(1)

    @pl.when(my == 1)
    def _():
        g0_copy(RT).start()

    @pl.when(my == 0)
    def _():
        g0_copy(0).start()

    for idx in range(2, _I_S7):
        main_start(idx)

    row8 = lax.broadcasted_iota(jnp.int32, (8, 128), 0)
    lane8 = lax.broadcasted_iota(jnp.int32, (8, 128), 1)
    lgrp = lane8 >> 3

    def group0_row(src, t0, t1):
        d = jnp.full((8, 128), NEG, jnp.float32)
        for b in range(t0 // TB, -(-t1 // TB)):
            f = _fold(src, max(t0, b * TB), min(t1, (b + 1) * TB))
            d = jnp.where(lgrp == b, _rmax(f), d)
        return _pick_diag(d)

    landed, done, acc = set(), set(), {}
    for idx in range(_I_C):
        main_wait(idx)
        j0, k, q, n = _DMAS[idx]
        landed.update(j * TG + SH + t for j in range(j0, j0 + k) for t in range(q, q + n))
        if idx == 0:
            for later in range(_I_S7, len(_DMAS)):
                main_start(later)
        if idx == _I_FWD:
            to_smem().wait()
            from_smem().start()
        if idx == _I_SMEM:
            from_smem().wait()
            landed.update(range(ST0, ST0 + ST))
        for b in range(NB, CSTART // TB):
            if b not in done and all(t in landed for t in range(b * TB, (b + 1) * TB)):
                done.add(b)
                g = b // NB
                r = _rmax(_fold(tile, b * TB, (b + 1) * TB))
                if g in acc or g == LAST:
                    acc[g] = jnp.where(lgrp == b % NB, r, acc.get(g, NEG))
                else:
                    acc[g] = jnp.broadcast_to(r, (8, 128))
        if idx == _I_G0:
            @pl.when(my == 1)
            def _():
                g0_copy(RT).wait()
                part[0] = group0_row(lambda t: g0buf[t], RT, R7)

            @pl.when(my == 0)
            def _():
                g0_copy(0).wait()
                part[0] = group0_row(lambda t: g0buf[t], 0, R7)
                pl.semaphore_wait(barrier, 1)
        if _I_S7 <= idx < _I_S7 + len(_BULK):
            lo, cnt = _BULK[idx - _I_S7]
            for g in range(lo, lo + cnt):
                if g == 0:
                    part[0] = jnp.maximum(part[0], group0_row(tile, R7, TG))
                else:
                    assert all(b in done for b in range(g * NB, (g + 1) * NB))
                    part[g] = _pick_diag(acc[g])
            rows_remote(lo, cnt, 1 + idx - _I_S7).start()
    assert len(done) == CSTART // TB - NB

    acc0 = acc[LAST]
    b0 = CSTART // TB

    def diag(b):
        return lane8 == row8 + 8 * (b % NB)

    main_wait(_I_C)
    low = jnp.where(lane8 == row8, acc0, NEG)
    anc = low
    folds, halves = [], []
    for b in range(b0, b0 + NC):
        h0 = _fold(tile, b * TB, b * TB + TB // 2)
        f = jnp.maximum(h0, _fold(tile, b * TB + TB // 2, (b + 1) * TB))
        folds.append(f)
        halves.append(h0)
        anc = jnp.where(diag(b), f, anc)
    part[LAST] = _pick_diag(acc0)
    rows_remote(LAST, 1, 3).start()
    for _ in range(5):
        anc = jnp.maximum(pltpu.roll(anc, 1, 0), low)

    def chain(v, n):
        for z in range(n):
            v = jnp.maximum(v, anc if z % 2 else low)
        return v

    main_wait(_I_C + 1)
    folds.append(_fold(tile, (b0 + NC) * TB, NT))
    d = acc0
    aux = []
    for j in range(2):
        d = chain(jnp.where(lgrp == (b0 + j) % NB, _rmax(folds[j]), d), 2)
        aux.append(jnp.where(diag(b0 + j), _rmax(halves[j]), NEG))
    for j in range(2, NC + NF):
        d = jnp.where(lane8 >= 8 * ((b0 + j) % NB), _rmax(folds[j]), d)
    own = _pick_diag(d)
    last_v[...] = own
    last_remote().start()
    aux = [chain(aux[0], 9), chain(aux[1], 7)]

    @pl.when(my == 1)
    def _():
        again = pltpu.make_async_copy(x_ref.at[pl.ds(0, RT)], rawbuf, lsem.at[3])
        again.start()
        raw_remote().wait_send()
        again.wait()

    @pl.when(my == 0)
    def _():
        raw_remote().wait_recv()

    own0 = jnp.maximum(part[0], group0_row(lambda t: rawbuf[t], 0, RT))
    own = jnp.maximum(own, jnp.max(jnp.maximum(aux[0], aux[1]), axis=0, keepdims=True))

    last_remote().wait_send()
    rows_remote(LAST, 1, 3).wait_send()
    for k, (lo, cnt) in enumerate(_BULK):
        rows_remote(lo, cnt, 1 + k).wait()
        for g in range(lo, lo + cnt):
            o_ref[g] = jnp.maximum(own0 if g == 0 else part[g], rbuf[g])

    rows_remote(LAST, 1, 3).wait_recv()
    own = jnp.maximum(own, rbuf[LAST])
    last_remote().wait_recv()
    lane = lax.broadcasted_iota(jnp.int32, (1, 128), 1)
    got = jnp.full((1, 128), NEG, jnp.float32)
    for i in range(G - KLAST, G):
        got = jnp.where(lane == i, last_s[0, i], got)
    o_ref[LAST] = jnp.maximum(own, got)


def _compiler_params():
    try:
        return pltpu.CompilerParams(collective_id=0, disable_semaphore_checks=True)
    except TypeError:
        return pltpu.CompilerParams(collective_id=0)


def pallas_dist_max_ax1_xy_m2048_n1024_kernel(x: jax.Array):
    tiles = x.reshape(M // 8, 8, TB, 128).transpose(0, 2, 1, 3).reshape(NT, 8, 128)
    out = pl.pallas_call(
        _body,
        out_shape=jax.ShapeDtypeStruct((NG, 1, 128), jnp.float32),
        in_specs=[pl.BlockSpec(memory_space=pl.ANY), pl.BlockSpec(memory_space=pl.ANY)],
        out_specs=pl.BlockSpec(memory_space=pltpu.VMEM),
        scratch_shapes=[
            pltpu.VMEM((NG, TG, 8, 128), jnp.float32),
            pltpu.VMEM((R7, 8, 128), jnp.float32),
            pltpu.VMEM((RT, 8, 128), jnp.float32),
            pltpu.VMEM((NG, 1, 128), jnp.float32),
            pltpu.VMEM((NG, 1, 128), jnp.float32),
            pltpu.VMEM((1, 128), jnp.float32),
            pltpu.SMEM((1, 128), jnp.float32),
            pltpu.SMEM((ST, 8, 128), jnp.float32),
            pltpu.SemaphoreType.DMA((len(_DMAS),)),
            pltpu.SemaphoreType.DMA((4,)),
            pltpu.SemaphoreType.DMA((5,)),
            pltpu.SemaphoreType.DMA((5,)),
        ],
        compiler_params=_compiler_params(),
    )(tiles.reshape(NG, TG, 8, 128), tiles)
    return out.reshape(M, 1)
```

```python
import functools

import jax
import jax.numpy as jnp
from jax import lax
from jax.experimental import pallas as pl
from jax.experimental.pallas import tpu as pltpu

M, N = 2048, 1024
G = 128
NG = M // G
NB = G // 8
TB = N // 128
TG = NB * TB
NT = NG * TG
LAST = NG - 1
NEG = float("-inf")
MESH = pl.DeviceIdType.MESH

U = 16
SH = 7
RT = 117
R7 = SH + 7 * U
QS = 2
ST0, ST = TG + SH, QS * U
QL = 3
NC, NF = 3, 1
CSTART = NT - (NC + NF) * TB
KLAST = 8 * (NC + NF)


def _plan():
    dmas = []
    for i in range(8):
        lo = 2 if i < QS else (1 if i < 7 else 0)
        hi = NG if i < QL else NG - 1
        splits = [hi - lo] if i < 7 else [7, 8]
        for k in splits:
            dmas.append((lo, k, i * U, U))
            lo += k
    c = CSTART - LAST * TG - SH
    dmas.append((LAST, 1, QL * U, c - QL * U))
    dmas.append((LAST, 1, c, NC * TB))
    dmas.append((LAST, 1, c + NC * TB, NF * TB))
    return dmas


_DMAS = _plan()
_I_FWD = 2
_I_G0 = 5
_I_SMEM = 6
_I_S7 = 7
_I_C = len(_DMAS) - 2
_BULK = ((0, 7), (7, 8))


def _tree_max(parts):
    while len(parts) > 1:
        nxt = [jnp.maximum(parts[i], parts[i + 1]) for i in range(0, len(parts) - 1, 2)]
        if len(parts) % 2:
            nxt.append(parts[-1])
        parts = nxt
    return parts[0]


def _fold(ref, t0, t1):
    return jnp.max(ref[pl.ds(t0, t1 - t0)], axis=0)


def _rmax(f):
    return jnp.max(f, axis=1, keepdims=True)


def _pick_diag(d):
    lane = lax.broadcasted_iota(jnp.int32, (8, 128), 1)
    rots = [d] + [pltpu.roll(d, 8 - s, 0) for s in range(1, 8)]
    t = [jnp.where((lane & 1) != 0, rots[2 * i + 1], rots[2 * i]) for i in range(4)]
    u = [jnp.where((lane & 2) != 0, t[2 * i + 1], t[2 * i]) for i in range(2)]
    return jnp.where((lane & 4) != 0, u[1], u[0])[0:1, :]


def _body(xg_ref, x_ref, o_ref, buf, g0buf, rawbuf, part, rbuf, last_v, last_s, sbuf,
          msem, lsem, ssem, rsem):
    def fold(t0, t1):
        j, q = divmod(t0 - SH, TG)
        n = min(t1 - t0, TG - q)
        f = _fold(buf.at[j], q, q + n)
        return f if n == t1 - t0 else jnp.maximum(f, fold(t0 + n, t1))

    def fold_tree(t0, t1):
        return _tree_max([buf[(t - SH) // TG, (t - SH) % TG] for t in range(t0, t1)])

    def main_start(idx):
        j0, k, q, n = _DMAS[idx]
        if SH + q + n <= TG:
            pltpu.make_async_copy(xg_ref.at[pl.ds(j0, k), pl.ds(SH + q, n)],
                                  buf.at[pl.ds(j0, k), pl.ds(q, n)], msem.at[idx]).start()
        else:
            for j in range(j0, j0 + k):
                pltpu.make_async_copy(x_ref.at[pl.ds(j * TG + SH + q, n)],
                                      buf.at[j, pl.ds(q, n)], msem.at[idx]).start()

    def main_wait(idx):
        j0, k, q, n = _DMAS[idx]
        dst = buf.at[pl.ds(j0, k), pl.ds(q, n)]
        pltpu.make_async_copy(dst, dst, msem.at[idx]).wait()

    main_start(0)

    mx = lax.axis_index("x")
    my = lax.axis_index("y")
    peer = (mx, 1 - my)
    barrier = pltpu.get_barrier_semaphore()
    pl.semaphore_signal(barrier, inc=1, device_id=peer, device_id_type=MESH)

    def remote(src, dst, k):
        return pltpu.make_async_remote_copy(src, dst, ssem.at[k], rsem.at[k],
                                            device_id=peer, device_id_type=MESH)

    def raw_remote():
        return remote(x_ref.at[pl.ds(0, RT)], rawbuf, 0)

    def rows_remote(lo, n, k):
        return remote(part.at[pl.ds(lo, n)], rbuf.at[pl.ds(lo, n)], k)

    def last_remote():
        return remote(last_v, last_s, 4)

    def to_smem():
        return pltpu.make_async_copy(x_ref.at[pl.ds(ST0, ST)], sbuf, lsem.at[0])

    def from_smem():
        return pltpu.make_async_copy(sbuf, buf.at[1, pl.ds(0, ST)], lsem.at[1])

    def g0_copy(t0):
        return pltpu.make_async_copy(x_ref.at[pl.ds(t0, R7 - t0)],
                                     g0buf.at[pl.ds(t0, R7 - t0)], lsem.at[2])

    @pl.when(my == 1)
    def _():
        pl.semaphore_wait(barrier, 1)
        raw_remote().start()

    to_smem().start()
    main_start(1)

    @pl.when(my == 1)
    def _():
        g0_copy(RT).start()

    @pl.when(my == 0)
    def _():
        g0_copy(0).start()

    for idx in range(2, _I_S7):
        main_start(idx)

    row8 = lax.broadcasted_iota(jnp.int32, (8, 128), 0)
    lane8 = lax.broadcasted_iota(jnp.int32, (8, 128), 1)
    lgrp = lane8 >> 3

    def group0_row(fold_fn, t0, t1):
        d = jnp.full((8, 128), NEG, jnp.float32)
        for b in range(t0 // TB, -(-t1 // TB)):
            f = fold_fn(max(t0, b * TB), min(t1, (b + 1) * TB))
            d = jnp.where(lgrp == b, _rmax(f), d)
        return _pick_diag(d)

    landed, done, acc = set(), set(), {}
    for idx in range(_I_C):
        main_wait(idx)
        j0, k, q, n = _DMAS[idx]
        landed.update(j * TG + SH + t for j in range(j0, j0 + k) for t in range(q, q + n))
        if idx == 0:
            for later in range(_I_S7, len(_DMAS)):
                main_start(later)
        if idx == _I_FWD:
            to_smem().wait()
            from_smem().start()
        if idx == _I_SMEM:
            from_smem().wait()
            landed.update(range(ST0, ST0 + ST))
        for b in range(NB, CSTART // TB):
            if b not in done and all(t in landed for t in range(b * TB, (b + 1) * TB)):
                done.add(b)
                g = b // NB
                r = _rmax(fold(b * TB, (b + 1) * TB))
                if g in acc or g == LAST:
                    acc[g] = jnp.where(lgrp == b % NB, r, acc.get(g, NEG))
                else:
                    acc[g] = jnp.broadcast_to(r, (8, 128))
        if idx == _I_G0:
            @pl.when(my == 1)
            def _():
                g0_copy(RT).wait()
                part[0] = group0_row(functools.partial(_fold, g0buf), RT, R7)

            @pl.when(my == 0)
            def _():
                g0_copy(0).wait()
                part[0] = group0_row(functools.partial(_fold, g0buf), 0, R7)
                pl.semaphore_wait(barrier, 1)
        if _I_S7 <= idx < _I_S7 + len(_BULK):
            lo, cnt = _BULK[idx - _I_S7]
            for g in range(lo, lo + cnt):
                if g == 0:
                    part[0] = jnp.maximum(part[0], group0_row(fold, R7, TG))
                else:
                    assert all(b in done for b in range(g * NB, (g + 1) * NB))
                    part[g] = _pick_diag(acc[g])
            rows_remote(lo, cnt, 1 + idx - _I_S7).start()
    assert len(done) == CSTART // TB - NB

    acc0 = acc[LAST]
    b0 = CSTART // TB

    def diag(b):
        return lane8 == row8 + 8 * (b % NB)

    main_wait(_I_C)
    low = jnp.where(lane8 == row8, acc0, NEG)
    anc = low
    folds, halves = [], []
    for b in range(b0, b0 + NC):
        h0 = fold_tree(b * TB, b * TB + TB // 2)
        f = jnp.maximum(h0, fold_tree(b * TB + TB // 2, (b + 1) * TB))
        folds.append(f)
        halves.append(h0)
        anc = jnp.where(diag(b), f, anc)
    part[LAST] = _pick_diag(acc0)
    rows_remote(LAST, 1, 3).start()
    for _ in range(5):
        anc = jnp.maximum(pltpu.roll(anc, 1, 0), low)

    def chain(v, n):
        for z in range(n):
            v = jnp.maximum(v, anc if z % 2 else low)
        return v

    main_wait(_I_C + 1)
    folds.append(fold_tree((b0 + NC) * TB, NT))
    d = acc0
    aux = []
    for j in range(2):
        d = chain(jnp.where(lgrp == (b0 + j) % NB, _rmax(folds[j]), d), 2)
        aux.append(jnp.where(diag(b0 + j), _rmax(halves[j]), NEG))
    for j in range(2, NC + NF):
        d = jnp.where(lane8 >= 8 * ((b0 + j) % NB), _rmax(folds[j]), d)
    own = _pick_diag(d)
    last_v[...] = own
    last_remote().start()
    aux = [chain(aux[0], 9), chain(aux[1], 7)]

    @pl.when(my == 1)
    def _():
        again = pltpu.make_async_copy(x_ref.at[pl.ds(0, RT)], rawbuf, lsem.at[3])
        again.start()
        raw_remote().wait_send()
        again.wait()

    @pl.when(my == 0)
    def _():
        raw_remote().wait_recv()

    own0 = jnp.maximum(part[0], group0_row(functools.partial(_fold, rawbuf), 0, RT))
    own = jnp.maximum(own, jnp.max(jnp.maximum(aux[0], aux[1]), axis=0, keepdims=True))

    last_remote().wait_send()
    rows_remote(LAST, 1, 3).wait_send()
    for k, (lo, cnt) in enumerate(_BULK):
        rows_remote(lo, cnt, 1 + k).wait()
        for g in range(lo, lo + cnt):
            o_ref[g] = jnp.maximum(own0 if g == 0 else part[g], rbuf[g])

    rows_remote(LAST, 1, 3).wait_recv()
    own = jnp.maximum(own, rbuf[LAST])
    last_remote().wait_recv()
    lane = lax.broadcasted_iota(jnp.int32, (1, 128), 1)
    got = jnp.full((1, 128), NEG, jnp.float32)
    for i in range(G - KLAST, G):
        got = jnp.where(lane == i, last_s[0, i], got)
    o_ref[LAST] = jnp.maximum(own, got)


def _compiler_params():
    try:
        return pltpu.CompilerParams(collective_id=0, disable_semaphore_checks=True)
    except TypeError:
        return pltpu.CompilerParams(collective_id=0)


def pallas_dist_max_ax1_xy_m2048_n1024_kernel(x: jax.Array):
    tiles = x.reshape(M // 8, 8, TB, 128).transpose(0, 2, 1, 3).reshape(NT, 8, 128)
    out = pl.pallas_call(
        _body,
        out_shape=jax.ShapeDtypeStruct((NG, 1, 128), jnp.float32),
        in_specs=[pl.BlockSpec(memory_space=pl.ANY), pl.BlockSpec(memory_space=pl.ANY)],
        out_specs=pl.BlockSpec(memory_space=pltpu.VMEM),
        scratch_shapes=[
            pltpu.VMEM((NG, TG, 8, 128), jnp.float32),
            pltpu.VMEM((R7, 8, 128), jnp.float32),
            pltpu.VMEM((RT, 8, 128), jnp.float32),
            pltpu.VMEM((NG, 1, 128), jnp.float32),
            pltpu.VMEM((NG, 1, 128), jnp.float32),
            pltpu.VMEM((1, 128), jnp.float32),
            pltpu.SMEM((1, 128), jnp.float32),
            pltpu.SMEM((ST, 8, 128), jnp.float32),
            pltpu.SemaphoreType.DMA((len(_DMAS),)),
            pltpu.SemaphoreType.DMA((4,)),
            pltpu.SemaphoreType.DMA((5,)),
            pltpu.SemaphoreType.DMA((5,)),
        ],
        compiler_params=_compiler_params(),
    )(tiles.reshape(NG, TG, 8, 128), tiles)
    return out.reshape(M, 1)
```

```python
import functools

import jax
import jax.numpy as jnp
from jax import lax
from jax.experimental import pallas as pl
from jax.experimental.pallas import tpu as pltpu

M, N = 2048, 1024
G = 128
NG = M // G
NB = G // 8
TB = N // 128
TG = NB * TB
NT = NG * TG
LAST = NG - 1
NEG = float("-inf")
MESH = pl.DeviceIdType.MESH

U = 16
SH = 7
RT = 117
R7 = SH + 7 * U
QS = 2
ST0, ST = TG + SH, QS * U
QL = 3
NC, NF = 3, 1
CSTART = NT - (NC + NF) * TB
KLAST = 8 * (NC + NF)


def _plan():
    dmas = []
    for i in range(8):
        lo = 2 if i < QS else (1 if i < 7 else 0)
        hi = NG if i < QL else NG - 1
        splits = [hi - lo] if i < 7 else [7, 8]
        for k in splits:
            dmas.append((lo, k, i * U, U))
            lo += k
    c = CSTART - LAST * TG - SH
    dmas.append((LAST, 1, QL * U, c - QL * U))
    dmas.append((LAST, 1, c, NC * TB))
    dmas.append((LAST, 1, c + NC * TB, NF * TB))
    return dmas


_DMAS = _plan()
_I_FWD = 2
_I_G0 = 5
_I_SMEM = 6
_I_S7 = 7
_I_C = len(_DMAS) - 2
_BULK = ((0, 7), (7, 8))


def _fold(ref, t0, t1):
    return jnp.max(ref[pl.ds(t0, t1 - t0)], axis=0)


def _rmax(f):
    return jnp.max(f, axis=1, keepdims=True)


def _pick_diag(d):
    lane = lax.broadcasted_iota(jnp.int32, (8, 128), 1)
    rots = [d] + [pltpu.roll(d, 8 - s, 0) for s in range(1, 8)]
    t = [jnp.where((lane & 1) != 0, rots[2 * i + 1], rots[2 * i]) for i in range(4)]
    u = [jnp.where((lane & 2) != 0, t[2 * i + 1], t[2 * i]) for i in range(2)]
    return jnp.where((lane & 4) != 0, u[1], u[0])[0:1, :]


def _body(xg_ref, x_ref, o_ref, buf, g0buf, rawbuf, part, rbuf, last_v, last_s, sbuf,
          msem, lsem, ssem, rsem):
    def fold(t0, t1):
        j, q = divmod(t0 - SH, TG)
        n = min(t1 - t0, TG - q)
        f = _fold(buf.at[j], q, q + n)
        return f if n == t1 - t0 else jnp.maximum(f, fold(t0 + n, t1))

    def main_start(idx):
        j0, k, q, n = _DMAS[idx]
        if SH + q + n <= TG:
            pltpu.make_async_copy(xg_ref.at[pl.ds(j0, k), pl.ds(SH + q, n)],
                                  buf.at[pl.ds(j0, k), pl.ds(q, n)], msem.at[idx]).start()
        else:
            for j in range(j0, j0 + k):
                pltpu.make_async_copy(x_ref.at[pl.ds(j * TG + SH + q, n)],
                                      buf.at[j, pl.ds(q, n)], msem.at[idx]).start()

    def main_wait(idx):
        j0, k, q, n = _DMAS[idx]
        dst = buf.at[pl.ds(j0, k), pl.ds(q, n)]
        pltpu.make_async_copy(dst, dst, msem.at[idx]).wait()

    main_start(0)

    mx = lax.axis_index("x")
    my = lax.axis_index("y")
    peer = (mx, 1 - my)
    barrier = pltpu.get_barrier_semaphore()
    pl.semaphore_signal(barrier, inc=1, device_id=peer, device_id_type=MESH)

    def remote(src, dst, k):
        return pltpu.make_async_remote_copy(src, dst, ssem.at[k], rsem.at[k],
                                            device_id=peer, device_id_type=MESH)

    def raw_remote():
        return remote(x_ref.at[pl.ds(0, RT)], rawbuf, 0)

    def rows_remote(lo, n, k):
        return remote(part.at[pl.ds(lo, n)], rbuf.at[pl.ds(lo, n)], k)

    def last_remote():
        return remote(last_v, last_s, 4)

    def to_smem():
        return pltpu.make_async_copy(x_ref.at[pl.ds(ST0, ST)], sbuf, lsem.at[0])

    def from_smem():
        return pltpu.make_async_copy(sbuf, buf.at[1, pl.ds(0, ST)], lsem.at[1])

    def g0_copy(t0):
        return pltpu.make_async_copy(x_ref.at[pl.ds(t0, R7 - t0)],
                                     g0buf.at[pl.ds(t0, R7 - t0)], lsem.at[2])

    @pl.when(my == 1)
    def _():
        pl.semaphore_wait(barrier, 1)
        raw_remote().start()

    to_smem().start()
    main_start(1)

    @pl.when(my == 1)
    def _():
        g0_copy(RT).start()

    @pl.when(my == 0)
    def _():
        g0_copy(0).start()

    for idx in range(2, _I_S7):
        main_start(idx)

    row8 = lax.broadcasted_iota(jnp.int32, (8, 128), 0)
    lane8 = lax.broadcasted_iota(jnp.int32, (8, 128), 1)
    lgrp = lane8 >> 3

    def group0_row(fold_fn, t0, t1):
        d = jnp.full((8, 128), NEG, jnp.float32)
        for b in range(t0 // TB, -(-t1 // TB)):
            f = fold_fn(max(t0, b * TB), min(t1, (b + 1) * TB))
            d = jnp.where(lgrp == b, _rmax(f), d)
        return _pick_diag(d)

    landed, done, acc = set(), set(), {}
    for idx in range(_I_C):
        main_wait(idx)
        j0, k, q, n = _DMAS[idx]
        landed.update(j * TG + SH + t for j in range(j0, j0 + k) for t in range(q, q + n))
        if idx == 0:
            for later in range(_I_S7, len(_DMAS)):
                main_start(later)
        if idx == _I_FWD:
            to_smem().wait()
            from_smem().start()
        if idx == _I_SMEM:
            from_smem().wait()
            landed.update(range(ST0, ST0 + ST))
        for b in range(NB, CSTART // TB):
            if b not in done and all(t in landed for t in range(b * TB, (b + 1) * TB)):
                done.add(b)
                g = b // NB
                r = _rmax(fold(b * TB, (b + 1) * TB))
                if g in acc or g == LAST:
                    acc[g] = jnp.where(lgrp == b % NB, r, acc.get(g, NEG))
                else:
                    acc[g] = jnp.broadcast_to(r, (8, 128))
        if idx == _I_G0:
            @pl.when(my == 1)
            def _():
                g0_copy(RT).wait()
                part[0] = group0_row(functools.partial(_fold, g0buf), RT, R7)

            @pl.when(my == 0)
            def _():
                g0_copy(0).wait()
                part[0] = group0_row(functools.partial(_fold, g0buf), 0, R7)
                pl.semaphore_wait(barrier, 1)
        if _I_S7 <= idx < _I_S7 + len(_BULK):
            lo, cnt = _BULK[idx - _I_S7]
            for g in range(lo, lo + cnt):
                if g == 0:
                    part[0] = jnp.maximum(part[0], group0_row(fold, R7, TG))
                else:
                    assert all(b in done for b in range(g * NB, (g + 1) * NB))
                    part[g] = _pick_diag(acc[g])
            rows_remote(lo, cnt, 1 + idx - _I_S7).start()
    assert len(done) == CSTART // TB - NB

    acc0 = acc[LAST]
    b0 = CSTART // TB

    def diag(b):
        return lane8 == row8 + 8 * (b % NB)

    main_wait(_I_C)
    low = jnp.where(lane8 == row8, acc0, NEG)
    anc = low
    folds, halves = [], []
    for b in range(b0, b0 + NC):
        h0 = fold(b * TB, b * TB + TB // 2)
        f = jnp.maximum(h0, fold(b * TB + TB // 2, (b + 1) * TB))
        folds.append(f)
        halves.append(h0)
        anc = jnp.where(diag(b), f, anc)
    part[LAST] = _pick_diag(acc0)
    rows_remote(LAST, 1, 3).start()
    for _ in range(5):
        anc = jnp.maximum(pltpu.roll(anc, 1, 0), low)

    def chain(v, n):
        for z in range(n):
            v = jnp.maximum(v, anc if z % 2 else low)
        return v

    main_wait(_I_C + 1)
    folds.append(fold((b0 + NC) * TB, NT))
    d = acc0
    aux = []
    for j in range(2):
        d = chain(jnp.where(lgrp == (b0 + j) % NB, _rmax(folds[j]), d), 2)
        aux.append(jnp.where(diag(b0 + j), _rmax(halves[j]), NEG))
    for j in range(2, NC + NF):
        d = jnp.where(lane8 >= 8 * ((b0 + j) % NB), _rmax(folds[j]), d)
    own = _pick_diag(d)
    last_v[...] = own
    last_remote().start()
    aux = [chain(aux[0], 9), chain(aux[1], 7)]

    @pl.when(my == 1)
    def _():
        again = pltpu.make_async_copy(x_ref.at[pl.ds(0, RT)], rawbuf, lsem.at[3])
        again.start()
        raw_remote().wait_send()
        again.wait()

    @pl.when(my == 0)
    def _():
        raw_remote().wait_recv()

    own0 = jnp.maximum(part[0], group0_row(functools.partial(_fold, rawbuf), 0, RT))
    own = jnp.maximum(own, jnp.max(jnp.maximum(aux[0], aux[1]), axis=0, keepdims=True))

    last_remote().wait_send()
    rows_remote(LAST, 1, 3).wait_send()
    for k, (lo, cnt) in enumerate(_BULK):
        rows_remote(lo, cnt, 1 + k).wait()
        for g in range(lo, lo + cnt):
            o_ref[g] = jnp.maximum(own0 if g == 0 else part[g], rbuf[g])

    rows_remote(LAST, 1, 3).wait_recv()
    own = jnp.maximum(own, rbuf[LAST])
    last_remote().wait_recv()
    lane = lax.broadcasted_iota(jnp.int32, (1, 128), 1)
    got = jnp.full((1, 128), NEG, jnp.float32)
    for i in range(G - KLAST, G):
        got = jnp.where(lane == i, last_s[0, i], got)
    o_ref[LAST] = jnp.maximum(own, got)


def _compiler_params():
    try:
        return pltpu.CompilerParams(collective_id=0, disable_semaphore_checks=True)
    except TypeError:
        return pltpu.CompilerParams(collective_id=0)


def pallas_dist_max_ax1_xy_m2048_n1024_kernel(x: jax.Array):
    tiles = x.reshape(M // 8, 8, TB, 128).transpose(0, 2, 1, 3).reshape(NT, 8, 128)
    out = pl.pallas_call(
        _body,
        out_shape=jax.ShapeDtypeStruct((NG, 1, 128), jnp.float32),
        in_specs=[pl.BlockSpec(memory_space=pl.ANY), pl.BlockSpec(memory_space=pl.ANY)],
        out_specs=pl.BlockSpec(memory_space=pltpu.VMEM),
        scratch_shapes=[
            pltpu.VMEM((NG, TG, 8, 128), jnp.float32),
            pltpu.VMEM((R7, 8, 128), jnp.float32),
            pltpu.VMEM((RT, 8, 128), jnp.float32),
            pltpu.VMEM((NG, 1, 128), jnp.float32),
            pltpu.VMEM((NG, 1, 128), jnp.float32),
            pltpu.VMEM((1, 128), jnp.float32),
            pltpu.SMEM((1, 128), jnp.float32),
            pltpu.SMEM((ST, 8, 128), jnp.float32),
            pltpu.SemaphoreType.DMA((len(_DMAS),)),
            pltpu.SemaphoreType.DMA((4,)),
            pltpu.SemaphoreType.DMA((5,)),
            pltpu.SemaphoreType.DMA((5,)),
        ],
        compiler_params=_compiler_params(),
    )(tiles.reshape(NG, TG, 8, 128), tiles)
    return out.reshape(M, 1)
```

```python
import functools

import jax
import jax.numpy as jnp
from jax import lax
from jax.experimental import pallas as pl
from jax.experimental.pallas import tpu as pltpu

M, N = 2048, 1024
G = 128
NG = M // G
NB = G // 8
TB = N // 128
TG = NB * TB
NT = NG * TG
LAST = NG - 1
NEG = float("-inf")
MESH = pl.DeviceIdType.MESH

U = 16
SH = 7
RT = 117
R7 = SH + 7 * U
QS = 2
ST0, ST = TG + SH, QS * U
QL = 3
NC, NF = 3, 1
CSTART = NT - (NC + NF) * TB
KLAST = 8 * (NC + NF)


def _plan():
    dmas = []
    for i in range(8):
        lo = 2 if i < QS else (1 if i < 7 else 0)
        hi = NG if i < QL else NG - 1
        splits = [hi - lo] if i < 7 else [7, 8]
        for k in splits:
            dmas.append((lo, k, i * U, U))
            lo += k
    c = CSTART - LAST * TG - SH
    dmas.append((LAST, 1, QL * U, c - QL * U))
    dmas.append((LAST, 1, c, NC * TB))
    dmas.append((LAST, 1, c + NC * TB, NF * TB))
    return dmas


_DMAS = _plan()
_I_FWD = 2
_I_G0 = 5
_I_SMEM = 6
_I_S7 = 7
_I_C = len(_DMAS) - 2
_BULK = ((0, 7), (7, 8))


def _fold(ref, t0, t1):
    return jnp.max(ref[pl.ds(t0, t1 - t0)], axis=0)


def _rmax(f):
    return jnp.max(f, axis=1, keepdims=True)


def _pick_diag(d):
    lane = lax.broadcasted_iota(jnp.int32, (8, 128), 1)
    rots = [d] + [pltpu.roll(d, 8 - s, 0) for s in range(1, 8)]
    t = [jnp.where((lane & 1) != 0, rots[2 * i + 1], rots[2 * i]) for i in range(4)]
    u = [jnp.where((lane & 2) != 0, t[2 * i + 1], t[2 * i]) for i in range(2)]
    return jnp.where((lane & 4) != 0, u[1], u[0])[0:1, :]


def _body(xg_ref, x_ref, o_ref, buf, g0buf, rawbuf, part, rbuf, last_v, last_s, sbuf,
          msem, lsem, ssem, rsem):
    def fold(t0, t1):
        j, q = divmod(t0 - SH, TG)
        n = min(t1 - t0, TG - q)
        f = _fold(buf.at[j], q, q + n)
        return f if n == t1 - t0 else jnp.maximum(f, fold(t0 + n, t1))

    def main_start(idx):
        j0, k, q, n = _DMAS[idx]
        if SH + q + n <= TG:
            pltpu.make_async_copy(xg_ref.at[pl.ds(j0, k), pl.ds(SH + q, n)],
                                  buf.at[pl.ds(j0, k), pl.ds(q, n)], msem.at[idx]).start()
        else:
            for j in range(j0, j0 + k):
                pltpu.make_async_copy(x_ref.at[pl.ds(j * TG + SH + q, n)],
                                      buf.at[j, pl.ds(q, n)], msem.at[idx]).start()

    def main_wait(idx):
        j0, k, q, n = _DMAS[idx]
        dst = buf.at[pl.ds(j0, k), pl.ds(q, n)]
        pltpu.make_async_copy(dst, dst, msem.at[idx]).wait()

    main_start(0)

    mx = lax.axis_index("x")
    my = lax.axis_index("y")
    peer = (mx, 1 - my)
    barrier = pltpu.get_barrier_semaphore()
    pl.semaphore_signal(barrier, inc=1, device_id=peer, device_id_type=MESH)

    def remote(src, dst, k):
        return pltpu.make_async_remote_copy(src, dst, ssem.at[k], rsem.at[k],
                                            device_id=peer, device_id_type=MESH)

    def raw_remote():
        return remote(x_ref.at[pl.ds(0, RT)], rawbuf, 0)

    def rows_remote(lo, n, k):
        return remote(part.at[pl.ds(lo, n)], rbuf.at[pl.ds(lo, n)], k)

    def last_remote():
        return remote(last_v, last_s, 4)

    def to_smem():
        return pltpu.make_async_copy(x_ref.at[pl.ds(ST0, ST)], sbuf, lsem.at[0])

    def from_smem():
        return pltpu.make_async_copy(sbuf, buf.at[1, pl.ds(0, ST)], lsem.at[1])

    def g0_copy(t0):
        return pltpu.make_async_copy(x_ref.at[pl.ds(t0, R7 - t0)],
                                     g0buf.at[pl.ds(t0, R7 - t0)], lsem.at[2])

    @pl.when(my == 1)
    def _():
        pl.semaphore_wait(barrier, 1)
        raw_remote().start()

    to_smem().start()
    main_start(1)

    @pl.when(my == 1)
    def _():
        g0_copy(RT).start()

    @pl.when(my == 0)
    def _():
        g0_copy(0).start()

    for idx in range(2, _I_S7):
        main_start(idx)

    row8 = lax.broadcasted_iota(jnp.int32, (8, 128), 0)
    lane8 = lax.broadcasted_iota(jnp.int32, (8, 128), 1)
    lgrp = lane8 >> 3

    def group0_row(fold_fn, t0, t1):
        d = jnp.full((8, 128), NEG, jnp.float32)
        for b in range(t0 // TB, -(-t1 // TB)):
            f = fold_fn(max(t0, b * TB), min(t1, (b + 1) * TB))
            d = jnp.where(lgrp == b, _rmax(f), d)
        return _pick_diag(d)

    landed, done, acc = set(), set(), {}
    for idx in range(_I_C):
        main_wait(idx)
        j0, k, q, n = _DMAS[idx]
        landed.update(j * TG + SH + t for j in range(j0, j0 + k) for t in range(q, q + n))
        if idx == 0:
            for later in range(_I_S7, len(_DMAS)):
                main_start(later)
        if idx == _I_FWD:
            to_smem().wait()
            from_smem().start()
        if idx == _I_SMEM:
            from_smem().wait()
            landed.update(range(ST0, ST0 + ST))
        for b in range(NB, CSTART // TB):
            if b not in done and all(t in landed for t in range(b * TB, (b + 1) * TB)):
                done.add(b)
                g = b // NB
                r = _rmax(fold(b * TB, (b + 1) * TB))
                if g in acc or g == LAST:
                    acc[g] = jnp.where(lgrp == b % NB, r, acc.get(g, NEG))
                else:
                    acc[g] = jnp.broadcast_to(r, (8, 128))
        if idx == _I_G0:
            @pl.when(my == 1)
            def _():
                g0_copy(RT).wait()
                part[0] = group0_row(functools.partial(_fold, g0buf), RT, R7)

            @pl.when(my == 0)
            def _():
                g0_copy(0).wait()
                part[0] = group0_row(functools.partial(_fold, g0buf), 0, R7)
                pl.semaphore_wait(barrier, 1)
        if _I_S7 <= idx < _I_S7 + len(_BULK):
            lo, cnt = _BULK[idx - _I_S7]
            for g in range(lo, lo + cnt):
                if g == 0:
                    part[0] = jnp.maximum(part[0], group0_row(fold, R7, TG))
                else:
                    assert all(b in done for b in range(g * NB, (g + 1) * NB))
                    part[g] = _pick_diag(acc[g])
            rows_remote(lo, cnt, 1 + idx - _I_S7).start()
    assert len(done) == CSTART // TB - NB

    acc0 = acc[LAST]
    b0 = CSTART // TB

    def diag(b):
        return lane8 == row8 + 8 * (b % NB)

    main_wait(_I_C)
    low = jnp.where(lane8 == row8, acc0, NEG)
    anc = low
    folds, halves = [], []
    for b in range(b0, b0 + NC):
        h0 = fold(b * TB, b * TB + TB // 2)
        f = jnp.maximum(h0, fold(b * TB + TB // 2, (b + 1) * TB))
        folds.append(f)
        halves.append(h0)
        anc = jnp.where(diag(b), f, anc)
    part[LAST] = _pick_diag(acc0)
    rows_remote(LAST, 1, 3).start()
    for _ in range(5):
        anc = jnp.maximum(pltpu.roll(anc, 1, 0), low)

    def chain(v, n):
        for z in range(n):
            v = jnp.maximum(v, anc if z % 2 else low)
        return v

    main_wait(_I_C + 1)
    folds.append(fold((b0 + NC) * TB, NT))
    d = acc0
    aux = []
    for j in range(2):
        d = chain(jnp.where(lgrp == (b0 + j) % NB, _rmax(folds[j]), d), 2)
        aux.append(jnp.where(diag(b0 + j), _rmax(halves[j]), NEG))
    for j in range(2, NC + NF):
        d = jnp.where(lane8 >= 8 * ((b0 + j) % NB), _rmax(folds[j]), d)
    own = _pick_diag(d)
    last_v[...] = own
    last_remote().start()
    aux = [chain(aux[0], 9), chain(aux[1], 7)]

    @pl.when(my == 1)
    def _():
        again = pltpu.make_async_copy(x_ref.at[pl.ds(0, RT)], rawbuf, lsem.at[3])
        again.start()
        raw_remote().wait_send()
        again.wait()

    @pl.when(my == 0)
    def _():
        raw_remote().wait_recv()

    own0 = jnp.maximum(part[0], group0_row(functools.partial(_fold, rawbuf), 0, RT))
    own = jnp.maximum(own, jnp.max(jnp.maximum(aux[0], aux[1]), axis=0, keepdims=True))

    last_remote().wait_send()
    rows_remote(LAST, 1, 3).wait_send()
    for k, (lo, cnt) in enumerate(_BULK):
        rows_remote(lo, cnt, 1 + k).wait()
        for g in range(lo, lo + cnt):
            o_ref[g] = jnp.maximum(own0 if g == 0 else part[g], rbuf[g])

    rows_remote(LAST, 1, 3).wait_recv()
    own = jnp.maximum(own, rbuf[LAST])
    last_remote().wait_recv()
    lane = lax.broadcasted_iota(jnp.int32, (1, 128), 1)
    got = jnp.full((1, 128), NEG, jnp.float32)
    for i in range(G - KLAST, G):
        got = jnp.where(lane == i, last_s[0, i], got)
    o_ref[LAST] = jnp.maximum(own, got)


def _scoped_body(*refs):
    pl.run_scoped(
        functools.partial(_body, *refs),
        pltpu.SemaphoreType.DMA((len(_DMAS),)),
        pltpu.SemaphoreType.DMA((4,)),
        pltpu.SemaphoreType.DMA((5,)),
        pltpu.SemaphoreType.DMA((5,)),
    )


def pallas_dist_max_ax1_xy_m2048_n1024_kernel(x: jax.Array):
    tiles = x.reshape(M // 8, 8, TB, 128).transpose(0, 2, 1, 3).reshape(NT, 8, 128)
    out = pl.pallas_call(
        _scoped_body,
        out_shape=jax.ShapeDtypeStruct((NG, 1, 128), jnp.float32),
        in_specs=[pl.BlockSpec(memory_space=pl.ANY), pl.BlockSpec(memory_space=pl.ANY)],
        out_specs=pl.BlockSpec(memory_space=pltpu.VMEM),
        scratch_shapes=[
            pltpu.VMEM((NG, TG, 8, 128), jnp.float32),
            pltpu.VMEM((R7, 8, 128), jnp.float32),
            pltpu.VMEM((RT, 8, 128), jnp.float32),
            pltpu.VMEM((NG, 1, 128), jnp.float32),
            pltpu.VMEM((NG, 1, 128), jnp.float32),
            pltpu.VMEM((1, 128), jnp.float32),
            pltpu.SMEM((1, 128), jnp.float32),
            pltpu.SMEM((ST, 8, 128), jnp.float32),
        ],
        compiler_params=pltpu.CompilerParams(collective_id=0),
    )(tiles.reshape(NG, TG, 8, 128), tiles)
    return out.reshape(M, 1)
```
